```python
import numpy as np

kernel_name = "dist_max_ax1_xy_m4096_n1024"

def setup_inputs():
    return {"x": np.random.randn(8192, 2048).astype(np.float32)}

def reference(x: np.ndarray) -> np.ndarray:
    return np.max(x, axis=1, keepdims=True)
```

```python
import jax
import jax.numpy as jnp
from jax import lax
from jax.experimental import pallas as pl
from jax.experimental.pallas import tpu as pltpu

_MESH = pl.DeviceIdType.MESH
_L = 128
_CHUNKS = (8, 8, 8, 4, 2, 1)
_TAIL = (96, 32)
_BULK = 30


def _colmax(buf, r0, rows):
    vs = [buf[pl.ds(r0, rows), c * _L:(c + 1) * _L] for c in range(buf.shape[1] // _L)]
    while len(vs) > 1:
        vs = [jnp.maximum(vs[i], vs[i + 1]) for i in range(0, len(vs), 2)]
    return vs[0]


def _block(buf, part, b):
    r0 = b * _L if isinstance(b, int) else pl.multiple_of(b * _L, _L)
    part[b] = jnp.max(_colmax(buf, r0, _L).T, axis=0, keepdims=True)


def pallas_dist_max_ax1_xy_m4096_n1024_kernel(x: jax.Array):
    m, n = x.shape
    nb = m // _L

    def body(x_hbm, o_ref, buf, part, recv, in_sems, ssem, rsem):
        loads, r = [], 0
        for k in [c * _L for c in _CHUNKS] + list(_TAIL):
            cp = pltpu.make_async_copy(x_hbm.at[pl.ds(r, k)], buf.at[pl.ds(r, k)], in_sems.at[len(loads)])
            cp.start()
            loads.append(cp)
            r += k
        peer = (lax.axis_index("x"), 1 - lax.axis_index("y"))
        bar = pltpu.get_barrier_semaphore()
        pl.semaphore_signal(bar, 1, device_id=peer, device_id_type=_MESH)
        pl.semaphore_wait(bar, 1)

        def swap(i, b0, b1):
            return pltpu.make_async_remote_copy(
                part.at[pl.ds(b0, b1 - b0)], recv.at[pl.ds(b0, b1 - b0)],
                ssem.at[i], rsem.at[i], device_id=peer, device_id_type=_MESH)

        bulk, last = swap(0, 0, _BULK), swap(1, _BULK, nb)
        b = 0
        for i, c in enumerate(_CHUNKS):
            loads[i].wait()
            if c == 1:
                _block(buf, part, b)
            else:
                lax.fori_loop(b, b + c, lambda j, _: _block(buf, part, j), None)
            b += c
            if b == _BULK:
                bulk.start()
        diag = lax.broadcasted_iota(jnp.int32, (8, _L), 1) - lax.broadcasted_iota(jnp.int32, (8, _L), 0)
        acc = jnp.full((8, _L), -jnp.inf, jnp.float32)
        o = 0
        for j, k in enumerate(_TAIL):
            loads[len(_CHUNKS) + j].wait()
            for _ in range(k // 8):
                v = jnp.max(_colmax(buf, (nb - 1) * _L + o, 8), axis=1, keepdims=True)
                acc = jnp.where(diag == o, v, acc)
                o += 8
        part[nb - 1] = jnp.max(acc, axis=0, keepdims=True)
        last.start()
        bulk.wait()
        lo, hi = pl.ds(0, _BULK), pl.ds(_BULK, nb - _BULK)
        o_ref[lo] = jnp.maximum(part[lo], recv[lo])
        last.wait()
        o_ref[hi] = jnp.maximum(part[hi], recv[hi])

    out = pl.pallas_call(
        body,
        in_specs=[pl.BlockSpec(memory_space=pl.ANY)],
        out_specs=pl.BlockSpec(memory_space=pltpu.VMEM),
        out_shape=jax.ShapeDtypeStruct((nb, 1, _L), x.dtype),
        scratch_shapes=[
            pltpu.VMEM((m, n), x.dtype),
            pltpu.VMEM((nb, 1, _L), x.dtype),
            pltpu.VMEM((nb, 1, _L), x.dtype),
            pltpu.SemaphoreType.DMA((len(_CHUNKS) + len(_TAIL),)),
            pltpu.SemaphoreType.DMA((2,)),
            pltpu.SemaphoreType.DMA((2,)),
        ],
        compiler_params=pltpu.CompilerParams(vmem_limit_bytes=32 << 20, collective_id=0),
    )(x)
    return out.reshape(m, 1)
```

```python
import jax
import jax.numpy as jnp
from jax import lax
from jax.experimental import pallas as pl
from jax.experimental.pallas import tpu as pltpu

_SUB, _LANE = 8, 128

_PANEL = 256
_SHIFT = 1
_RELAY = 48
_EARLY = 80
_RELAY_DONE = 6
_LAST = 40
_WINDOW = 8


def _row_max(tiles):
    parts = [tiles[:, c] for c in range(tiles.shape[1])]
    while len(parts) > 1:
        parts = [jnp.maximum(a, b) for a, b in zip(parts[::2], parts[1::2])]
    return jnp.max(parts[0], axis=2, keepdims=True)


def _kernel(x_hbm, out, buf, relay, acc, mine, theirs, last_mine, last_theirs,
            load_sems, relay_sem, send_sems, recv_sems):
    panels = x_hbm.shape[0]
    blocks = out.shape[0]
    groups = _PANEL // _SUB
    neg_inf = jnp.array(-jnp.inf, out.dtype)

    run_end = _SUB - _SHIFT
    boxes = [
        (pl.ds(1, panels - 1), pl.ds(0, run_end)),
        (pl.ds(0, panels - 1), pl.ds(_PANEL - _SHIFT, _SHIFT)),
    ]
    for g in range(1, groups):
        count = panels - 1 if g <= groups // 2 else panels - 2
        boxes.append((pl.ds(1, count), pl.ds(g * _SUB - _SHIFT, _SUB)))
    boxes.append((panels - 1, pl.ds(_LANE + run_end, _LANE - _LAST)))
    boxes.append((panels - 1, pl.ds(_PANEL - _LAST + run_end, _LAST - run_end)))
    loads = [
        pltpu.make_async_copy(x_hbm.at[box], buf.at[box], load_sems.at[i % _WINDOW])
        for i, box in enumerate(boxes)
    ]

    def wait_load(i):
        loads[i].wait()
        if i + _WINDOW < len(loads):
            loads[i + _WINDOW].start()

    relayed = (0, pl.ds(0, _RELAY))
    to_smem = pltpu.make_async_copy(x_hbm.at[relayed], relay, relay_sem)
    from_smem = pltpu.make_async_copy(relay, buf.at[relayed], relay_sem)
    loads[0].start()
    to_smem.start()

    peer = (lax.axis_index("x"), 1 - lax.axis_index("y"))
    barrier = pltpu.get_barrier_semaphore()
    pl.semaphore_signal(
        barrier, 1, device_id=peer, device_id_type=pl.DeviceIdType.MESH)
    for load in loads[1:_WINDOW]:
        load.start()
    pl.semaphore_wait(barrier, 1)

    def to_peer(i, src, dst):
        return pltpu.make_async_remote_copy(
            src, dst, send_sems.at[i], recv_sems.at[i],
            device_id=peer, device_id_type=pl.DeviceIdType.MESH)

    early = (0, pl.ds(_RELAY, _EARLY - _RELAY))
    late = (0, pl.ds(_EARLY, _PANEL - _SHIFT - _EARLY))
    side, bulk, tail = pl.ds(0, 2), pl.ds(2, blocks - 3), pl.ds(blocks - 1, 1)
    swap_early = to_peer(0, x_hbm.at[early], buf.at[early])
    swap_late = to_peer(1, x_hbm.at[late], buf.at[late])
    swap_bulk = to_peer(2, mine.at[bulk], theirs.at[bulk])
    swap_side = to_peer(3, mine.at[side], theirs.at[side])
    swap_tail = to_peer(4, mine.at[tail], theirs.at[tail])
    swap_last = to_peer(5, last_mine, last_theirs)
    swap_early.start()

    diagonal = (lax.broadcasted_iota(jnp.int32, (_SUB, _LANE), 1)
                - lax.broadcasted_iota(jnp.int32, (_SUB, _LANE), 0))

    def reduce_group(g):
        half, lane = divmod(g * _SUB, _LANE)
        some = pl.ds(1, panels - 1 - half)
        maxima = _row_max(buf[some, pl.ds(g * _SUB, _SUB)])
        spread = jnp.where(diagonal == lane, maxima, acc[some] if lane else neg_inf)
        if lane + _SUB < _LANE:
            acc[some] = spread
        else:
            dense = jnp.max(spread, axis=1, keepdims=True)
            for p in range(some.size):
                mine[2 * (p + 1) + half] = dense[p]

    def reduce_rows(panel, start, rows):
        tiles = buf[panel, pl.ds(start, rows)]
        maxima = _row_max(tiles.reshape(rows // _SUB, _SUB, _SUB, _LANE))
        spread = neg_inf
        for g in range(rows // _SUB):
            lane = (start + g * _SUB) % _LANE
            spread = jnp.where(diagonal == lane, maxima[g], spread)
        return jnp.max(spread, axis=0, keepdims=True)

    wait_load(0)
    wait_load(1)
    for g in range(1, groups):
        if g == _RELAY_DONE:
            to_smem.wait()
            swap_late.start()
            from_smem.start()
        wait_load(g + 1)
        reduce_group(g - 1)
    reduce_group(groups - 1)
    swap_bulk.start()

    from_smem.wait()
    swap_early.wait_recv()
    swap_late.wait_recv()
    mine[0] = reduce_rows(0, 0, _LANE)
    mine[1] = reduce_rows(0, _LANE, _LANE)
    swap_side.start()

    wait_load(groups + 1)
    mine[blocks - 1] = reduce_rows(panels - 1, _LANE, _LANE - _LAST)
    swap_tail.start()
    wait_load(groups + 2)
    last_mine[...] = reduce_rows(panels - 1, _PANEL - _LAST, _LAST)
    swap_last.start()

    swap_early.wait_send()
    swap_late.wait_send()
    swap_bulk.wait()
    out[bulk] = jnp.maximum(mine[bulk], theirs[bulk])
    swap_side.wait()
    out[side] = jnp.maximum(mine[side], theirs[side])
    swap_tail.wait()
    swap_last.wait_send()
    result = jnp.maximum(
        jnp.maximum(mine[blocks - 1], theirs[blocks - 1]), last_mine[...])
    swap_last.wait_recv()
    lanes = lax.broadcasted_iota(jnp.int32, (1, _LANE), 1)
    chains = [neg_inf, neg_inf]
    for lane in range(_LANE - _LAST, _LANE):
        chains[lane % 2] = jnp.where(
            lanes == lane, last_theirs[0, lane], chains[lane % 2])
    out[blocks - 1] = jnp.maximum(jnp.maximum(result, chains[0]), chains[1])


def pallas_dist_max_ax1_xy_m4096_n1024_kernel(x: jax.Array):
    m, n = x.shape
    assert n == _SUB * _LANE and m % _PANEL == 0
    panels, blocks = m // _PANEL, m // _LANE
    tiles = x.reshape(m // _SUB, _SUB, n // _LANE, _LANE).transpose(0, 2, 1, 3)
    tiles = tiles.reshape(panels, _PANEL, _SUB, _LANE)
    out = pl.pallas_call(
        _kernel,
        out_shape=jax.ShapeDtypeStruct((blocks, 1, _LANE), x.dtype),
        in_specs=[pl.BlockSpec(memory_space=pl.ANY)],
        out_specs=pl.BlockSpec(memory_space=pltpu.VMEM),
        scratch_shapes=[
            pltpu.VMEM(tiles.shape, x.dtype),
            pltpu.SMEM((_RELAY, _SUB, _LANE), x.dtype),
            pltpu.VMEM((panels, _SUB, _LANE), x.dtype),
            pltpu.VMEM((blocks, 1, _LANE), x.dtype),
            pltpu.VMEM((blocks, 1, _LANE), x.dtype),
            pltpu.VMEM((1, _LANE), x.dtype),
            pltpu.SMEM((1, _LANE), x.dtype),
            pltpu.SemaphoreType.DMA((_WINDOW,)),
            pltpu.SemaphoreType.DMA,
            pltpu.SemaphoreType.DMA((6,)),
            pltpu.SemaphoreType.DMA((6,)),
        ],
        compiler_params=pltpu.CompilerParams(
            collective_id=0,
            vmem_limit_bytes=32 * 1024 * 1024,
            disable_semaphore_checks=True,
        ),
    )(tiles)
    return out.reshape(m, 1)
```
